```python
import numpy as np

kernel_name = "dist_sparse_attn_localglobal_qseq_kvseq_b2_sq128_skv128_hq4_dh64"

def setup_inputs():
    x = np.random.randn(2, 512, 512).astype(np.float32)
    Wq = np.random.randn(512, 256).astype(np.float32) * 0.02
    K_ext = np.random.randn(2, 512, 4, 64).astype(np.float32)
    V_ext = np.random.randn(2, 512, 4, 64).astype(np.float32)
    Wo = np.random.randn(256, 512).astype(np.float32) * 0.02
    return {"x": x, "Wq": Wq, "K_ext": K_ext, "V_ext": V_ext, "Wo": Wo}

def reference(x, Wq, K_ext, V_ext, Wo):
    B, Sq, Skv, Hq, Dh = 2, 512, 512, 4, 64
    Q = (x @ Wq).reshape(B, Sq, Hq, Dh)
    qi = np.arange(Sq)[:, None]
    ki = np.arange(Skv)[None, :]
    local = np.abs(qi - ki) <= 128
    glob = (ki < 32) | (qi < 32)
    mask = local | glob
    scores = np.einsum('bihd,bjhd->bhij', Q, K_ext).astype(np.float32) * 0.125
    scores = np.where(mask[None, None, :, :], scores, -1e9)
    scores_max = scores.max(axis=-1, keepdims=True)
    w = np.exp(scores - scores_max)
    row_keep = mask.any(axis=1)
    w_sum = np.where(row_keep[None, None, :, None], w.sum(axis=-1, keepdims=True), 1.0)
    w = w / w_sum
    w = np.where(row_keep[None, None, :, None], w, 0.0)
    ctx = np.einsum('bhij,bjhd->bihd', w, V_ext).reshape(B, Sq, Hq * Dh)
    return ctx @ Wo
```

```python
import jax
import jax.numpy as jnp
from jax import lax
from jax.experimental import pallas as pl
from jax.experimental.pallas import tpu as pltpu

F32 = jnp.float32
BF16 = jnp.bfloat16
U32 = jnp.uint32
T = 128
NG = 32
LOG2E = 1.4426950408889634
NEG = -1e9 * LOG2E
RLY = 96
RLY2 = 112
GCUT = 56
CUTS = (0, 8, 40, 128)
QSCALE = 0.125 * LOG2E
NP = len(CUTS) - 1
CUTS2 = (0, 32, 128)
A, B, C, D = 0, 1, 2, 3
MESH = pl.DeviceIdType.MESH


def _iota(shape, dim):
    return lax.broadcasted_iota(jnp.int32, shape, dim)


def _nn(a, b):
    return jnp.dot(a.astype(BF16), b, preferred_element_type=F32)


def _nt(a, b):
    return lax.dot_general(a.astype(BF16), b, (((1,), (1,)), ((), ())), preferred_element_type=F32)


class _Packed:
    def __init__(self, ref):
        self.ref = ref

    def _ix(self, idx):
        idx = idx if isinstance(idx, tuple) else (idx,)
        row = len(self.ref.shape) - 2
        out = []
        for ax, i in enumerate(idx):
            if ax == row and isinstance(i, slice):
                i = slice(None if i.start is None else i.start // 2, None if i.stop is None else i.stop // 2)
            out.append(i)
        return tuple(out)

    def __getitem__(self, idx):
        return pltpu.bitcast(self.ref[self._ix(idx)], BF16)

    def __setitem__(self, idx, val):
        self.ref[self._ix(idx)] = pltpu.bitcast(val, U32)

    def at(self, *idx):
        return self.ref.at[self._ix(idx)] if idx else self.ref


def _stack_heads(q):
    w = pltpu.bitcast(q, U32)
    lo = _iota(w.shape, 1) < 64
    z = jnp.zeros_like(w)
    return jnp.concatenate(
        [pltpu.bitcast(jnp.where(lo, w, z), BF16), pltpu.bitcast(jnp.where(lo, z, w), BF16)], axis=0)


def _pair(v):
    r = v.shape[0] // 2
    lo = _iota((r, T), 1) < 64
    return jnp.where(lo, v[:r], v[r:])


def _mask(kind, r):
    i = _iota((2 * r, T), 0)
    i = jnp.where(i >= r, i - r, i)
    j = _iota((2 * r, T), 1)
    if kind == "left":
        return j >= i
    if kind == "left_g":
        return (j >= i) | (j < NG)
    if kind == "right":
        return j <= i
    if kind == "right_g":
        return (j <= i) | (i < NG)
    if kind == "glob":
        return j < NG
    raise ValueError(kind)


def _softmax(tiles):
    mx = tiles[0]
    for s in tiles[1:]:
        mx = jnp.maximum(mx, s)
    m = jnp.max(mx, axis=1, keepdims=True)
    ps = [jnp.exp2(s - m) for s in tiles]
    tot = ps[0]
    for p in ps[1:]:
        tot = tot + p
    l = jnp.sum(tot, axis=1, keepdims=True)
    return ps, m, l


def _pack_glob(k, v):
    kw = pltpu.bitcast(k, U32)
    vw = pltpu.bitcast(v, U32)
    lane = _iota((32, T), 1)
    g = jnp.where(
        lane < 32, kw[:32],
        jnp.where(lane < 64, pltpu.roll(vw[:32], 32, 1),
                  jnp.where(lane < 96, pltpu.roll(kw[32:], 64, 1), pltpu.roll(vw[32:], 96, 1))))
    return pltpu.bitcast(g, BF16)


def _unpack_glob(g):
    w = pltpu.bitcast(g, U32)
    kg = jnp.concatenate([w, pltpu.roll(w, 64, 1)], axis=0)
    vg = jnp.concatenate([pltpu.roll(w, 96, 1), pltpu.roll(w, 32, 1)], axis=0)
    return pltpu.bitcast(kg, BF16), pltpu.bitcast(vg, BF16)


def _pack96(k, v):
    kw = pltpu.bitcast(k, U32)
    vw = pltpu.bitcast(v, U32)
    lo = _iota((32, T), 1) < NG
    vo = vw[32:]
    t1 = jnp.where(lo, pltpu.roll(vo, 96, 1), kw[:32])
    t2 = jnp.where(lo, pltpu.roll(vo, 64, 1), kw[32:])
    t3 = jnp.where(lo, pltpu.roll(vo, 32, 1), vw[:32])
    return [pltpu.bitcast(t, BF16) for t in (t1, t2, t3)]


def _unpack96_k(t1, t2, kg):
    w = jnp.concatenate([pltpu.bitcast(t1, U32), pltpu.bitcast(t2, U32)], axis=0)
    return pltpu.bitcast(jnp.where(_iota((64, T), 1) < NG, pltpu.bitcast(kg, U32), w), BF16)


def _unpack96_vo(t1, t2, vg):
    lane = _iota((32, T), 1)
    return jnp.where(
        lane < 32, pltpu.bitcast(vg, U32)[32:],
        jnp.where(lane < 64, pltpu.roll(pltpu.bitcast(t1, U32), 32, 1),
                  pltpu.roll(pltpu.bitcast(t2, U32), 64, 1)))


def _unpack96_v(t3, v_o, vg):
    w3 = pltpu.bitcast(t3, U32)
    lane = _iota((32, T), 1)
    ve = jnp.where(lane < 32, pltpu.bitcast(vg, U32)[:32], w3)
    vo = jnp.where(lane < 96, v_o, pltpu.roll(w3, 96, 1))
    return pltpu.bitcast(jnp.concatenate([ve, vo], axis=0), BF16)


def _weights(m, l, lses):
    mm = m
    for lse in lses:
        mm = jnp.maximum(mm, lse)
    w0 = jnp.exp2(m - mm)
    ws = [jnp.exp2(lse - mm) for lse in lses]
    den = w0 * l
    for w in ws:
        den = den + w
    inv = 1.0 / den
    return w0 * inv, [w * inv for w in ws]


def _nt2(p, v):
    r = p.shape[0] // 2
    return jnp.concatenate([_nt(p[:r], v), _nt(p[r:], v)], axis=0)


def _nn2(q, k):
    r = q.shape[0] // 2
    return jnp.concatenate([_nn(q[:r], k), _nn(q[r:], k)], axis=0)


def _fold(v):
    seg = (_iota((8, T), 1) % 64) // 2
    f = v[0:8]
    for k in range(1, v.shape[0] // 8):
        f = jnp.where(seg == k, v[8 * k:8 * k + 8], f)
    return f


def _unfold(f, rows):
    idx = jnp.where(_iota((8, T), 1) < 64, 0, 64)
    return jnp.concatenate(
        [jnp.take_along_axis(f, idx + 2 * k, axis=1) for k in range(rows // 8)], axis=0)


def _fold2(v):
    lane = _iota((8, T), 1)
    f = v[0:8]
    for k in range(1, 16):
        f = jnp.where(lane % 16 == k, v[8 * k:8 * k + 8], f)
    q = (lane % 64) // 16
    g = jnp.where(q == 0, f, jnp.where(
        q == 1, pltpu.roll(f, 6, 0), jnp.where(q == 2, pltpu.roll(f, 4, 0), pltpu.roll(f, 2, 0))))
    return g[0:2]


def _unfold2(r0, r1):
    sub = _iota((8, T), 0)
    h = jnp.where(sub % 2 == 0, jnp.broadcast_to(r0, (8, T)), jnp.broadcast_to(r1, (8, T)))
    idx = jnp.where(_iota((8, T), 1) < 64, 0, 64) + 16 * (sub // 2)
    return jnp.concatenate([jnp.take_along_axis(h, idx + k, axis=1) for k in range(16)], axis=0)


def _body(x_hbm, wq_hbm, k_hbm, v_hbm, wo_hbm, out,
          xf, wqf, wof, kvf, wqb, wob, kv, kvl, kvr, qp, q0, q0g, gbuf, gsend,
          st10, r0, lse3, o3, t96, qn, sts, str_, rs, rr,
          lsem, ssem, rsem, ent):
    me = lax.axis_index("i")
    bar = pltpu.get_barrier_semaphore()
    (wqb, wob, kv, kvl, kvr, qp, q0, q0g, gbuf, gsend, r0, o3, t96, qn, rs, rr) = map(
        _Packed, (wqb, wob, kv, kvl, kvr, qp, q0, q0g, gbuf, gsend, r0, o3, t96, qn, rs, rr))

    def ld(name):
        kind = name[0]
        if kind in ("k", "v"):
            c = name[1]
            src = (k_hbm if kind == "k" else v_hbm).at[pl.ds(c * T, T)]
            j = 0 if kind == "k" else 1
            return pltpu.make_async_copy(src, kvf.at[c, j], lsem.at[2 * c + j])
        if kind == "kp":
            _, c, n = name
            lo, hi = CUTS[n], CUTS[n + 1]
            return pltpu.make_async_copy(
                k_hbm.at[pl.ds(c * T + lo, hi - lo)], kvf.at[c, 0, pl.ds(lo, hi - lo)],
                lsem.at[13 + n + 2 * (c % 2) if n else 2 * c])
        if kind == "kq":
            _, c, n = name
            lo, hi = CUTS2[n], CUTS2[n + 1]
            return pltpu.make_async_copy(
                k_hbm.at[pl.ds(c * T + lo, hi - lo)], kvf.at[c, 0, pl.ds(lo, hi - lo)],
                lsem.at[14 if n else 2 * c])
        if kind == "wqh":
            h = name[1]
            return pltpu.make_async_copy(
                wq_hbm.at[:, pl.ds(h * T, T)], wqf.at[h], lsem.at[(10, 13)[h]])
        if kind == "x":
            return pltpu.make_async_copy(x_hbm.at[name[1]], xf.at[name[1]], lsem.at[8 + name[1]])
        if kind == "x0a":
            return pltpu.make_async_copy(x_hbm.at[0, pl.ds(0, NG)], xf.at[0, pl.ds(0, NG)], lsem.at[8])
        if kind == "x0b":
            return pltpu.make_async_copy(
                x_hbm.at[0, pl.ds(NG, T - NG)], xf.at[0, pl.ds(NG, T - NG)], lsem.at[12])
        return pltpu.make_async_copy(wo_hbm, wof, lsem.at[11])

    def ldwait(*name):
        ld(name).wait()

    def semwait(s, n):
        pl.semaphore_wait(s, n)

    def cast_kv(j, c):
        ldwait("kv"[j], c)
        kv[c, j] = kvf[c, j].astype(BF16)

    def cast_k_part(c, n):
        ldwait("kp", c, n)
        rows = slice(CUTS[n], CUTS[n + 1])
        kv[c, 0, rows] = kvf[c, 0, rows].astype(BF16)

    def cast_k_part2(c, n):
        ldwait("kq", c, n)
        rows = slice(CUTS2[n], CUTS2[n + 1])
        kv[c, 0, rows] = kvf[c, 0, rows].astype(BF16)

    def rc_desc(name, dst):
        kind = name[0]
        if kind == "L":
            _, j, c = name
            s, d, i = kv.at(c, j), kvl.at(c, j), 2 * c + j
        elif kind == "R":
            _, j, c = name
            s, d, i = kv.at(c, j), kvr.at(c, j), 8 + 2 * c + j
        elif kind == "Rp":
            _, c, n = name
            rows = slice(CUTS[n], CUTS[n + 1])
            s, d, i = kv.at(c, 0, rows), kvr.at(c, 0, rows), (43 + n if n else 8 + 2 * c)
        elif kind == "Lp":
            _, c, n = name
            rows = slice(CUTS2[n], CUTS2[n + 1])
            s, d, i = kv.at(c, 0, rows), kvl.at(c, 0, rows), (48 + n if n else 2 * c)
        elif kind == "g":
            s, d, i = gsend.at(name[1]), gbuf.at(name[1]), 16 + name[1]
        elif kind == "gf":
            s, d, i = gbuf.at(name[1]), gbuf.at(name[1]), 16 + name[1]
        elif kind == "q0":
            s, d, i = qp.at(name[1]), q0.at(name[1] - C), 20 + name[1] - C
        elif kind == "q0g":
            s, d, i = q0g.at(), q0g.at(), 22
        elif kind == "st10":
            s, d, i = st10, st10, 23
        elif kind == "r0d":
            s, d, i = r0.at(1), r0.at(1), 24
        elif kind == "r0c_hi":
            s, d, i = r0.at(0, slice(NG, T)), r0.at(0, slice(NG, T)), 25
        elif kind == "r0c_lo":
            s, d, i = r0.at(0, slice(0, NG)), r0.at(0, slice(0, NG)), 28
        elif kind == "lse3":
            s, d, i = lse3.at[name[1]], lse3.at[name[1]], 26 + name[1]
        elif kind == "o3":
            s, d, i = o3.at(name[1]), o3.at(name[1]), 30 + name[1]
        elif kind == "t12":
            s, d, i = t96.at(slice(0, 2)), t96.at(slice(0, 2)), 34
        elif kind == "t3":
            s, d, i = t96.at(2), t96.at(2), 35
        elif kind == "q":
            _, side, c = name
            s, d, i = qp.at(c), qn.at(side), 36 + side
        elif kind == "st":
            side = name[1]
            s, d, i = sts.at[1 - side], str_.at[side], 38 + side
        elif kind == "r":
            _, side, h = name
            rows = slice(64 * h, 64 * h + 64)
            s, d, i = rs.at(1 - side, rows), rr.at(side, rows), 40 + 2 * side + h
        elif kind == "ga":
            s, d, i = gbuf.at(A, slice(0, GCUT)), gbuf.at(A, slice(0, GCUT)), 16 + A
        elif kind == "gb":
            s, d, i = gsend.at(A, slice(GCUT, 64)), gbuf.at(A, slice(GCUT, 64)), 46
        elif kind == "rm":
            s, d, i = rs.at(1, slice(64, RLY)), rr.at(0, slice(64, RLY)), 41
        elif kind == "rr":
            s, d, i = rs.at(1, slice(RLY, T)), rs.at(1, slice(RLY, T)), 47
        elif kind == "rf":
            s, d, i = rs.at(1, slice(RLY, T)), rr.at(0, slice(RLY, T)), 48
        elif kind == "r2m":
            s, d, i = rs.at(0, slice(64, RLY2)), rr.at(1, slice(64, RLY2)), 43
        elif kind == "r2r":
            s, d, i = rs.at(0, slice(RLY2, T)), rr.at(1, slice(RLY2, T)), 51
        elif kind == "r2f":
            s, d, i = rr.at(1, slice(RLY2, T)), rr.at(1, slice(RLY2, T)), 52
        elif kind == "Lh":
            rows = slice(64 * name[1], 64 * name[1] + 64)
            s, d, i = kv.at(A, 1, rows), kvl.at(A, 1, rows), (2 * A + 1, 50)[name[1]]
        else:
            raise ValueError(name)
        return pltpu.make_async_remote_copy(
            src_ref=s, dst_ref=d, send_sem=ssem.at[i], recv_sem=rsem.at[i],
            device_id=(dst,), device_id_type=MESH)

    class Prog:
        def __init__(self):
            self.sent = []

        def send(self, name, dst):
            rc_desc(name, dst).start()
            self.sent.append((name, dst))

        def recv(self, *names):
            for n in names:
                rc_desc(n, 0).wait_recv()

        def drain(self, keep=()):
            for n, d in self.sent:
                if n not in keep:
                    rc_desc(n, d).wait_send()
            self.sent = [(n, d) for n, d in self.sent if n in keep]

    def cast_wq(*halves):
        for h in halves:
            ldwait("wqh", h)
            wqb[:, h * T:(h + 1) * T] = wqf[h].astype(BF16)

    def cast_wo():
        ldwait("wo")
        wob[...] = wof[...].astype(BF16)

    def qrows(xv):
        return (_nn(xv.astype(BF16), wqb[...]) * QSCALE).astype(BF16)

    def qproj(b):
        q = qrows(xf[b])
        qp[2 * b] = q[:, :T]
        qp[2 * b + 1] = q[:, T:]

    def wo_rows(c):
        return wob[(c % 2) * T:(c % 2 + 1) * T]

    def oproj_first(c, cx):
        out[c // 2] = _nn(cx, wo_rows(c))

    def oproj_add(c, cx):
        out[c // 2] = out[c // 2] + _nn(cx, wo_rows(c))

    def oproj_both(b, c0, c1):
        out[b] = _nn(jnp.concatenate([c0, c1], axis=1), wob[...])

    def norm(acc, l):
        return (acc * (1.0 / l)).astype(BF16)

    def masked(s, kind):
        return jnp.where(_mask(kind, s.shape[0] // 2), s, NEG)

    def qpair(c):
        h = c % 2
        qp[c] = (_nn(xf[c // 2], wqb[:, h * T:(h + 1) * T]) * QSCALE).astype(BF16)

    def helper_front(side, tiles):
        qm = _stack_heads(qn[side])
        ps, m, l = _softmax([masked(_nn2(qm, k), kind) for k, kind in tiles])
        sts[side] = _fold2(_pair(m + jnp.log2(l)))
        return ps, _pair(l)

    def helper(side, tiles):
        ps, l = helper_front(side, [(k, kind) for k, _, kind in tiles])
        acc = _nt2(ps[0], tiles[0][1])
        for pr, (_, v, _) in zip(ps[1:], tiles[1:]):
            acc = acc + _nt2(pr, v)
        rs[side] = norm(_pair(acc), l)

    def send_back(p, side, dst):
        p.send(("st", 1 - side), dst)
        p.send(("r", 1 - side, 0), dst)
        p.send(("r", 1 - side, 1), dst)

    def peer_lse(side):
        return _unfold2(str_[side, 0:1], str_[side, 1:2])

    def merge_rows(c, h, base, parts):
        rows = slice(64 * h, 64 * h + 64)
        cx = base[rows]
        for side, w in parts:
            cx = cx + w[rows] * rr[side, rows].astype(F32)
        out[c // 2, rows] = out[c // 2, rows] + _nn(cx, wo_rows(c))

    def diag_only(c):
        ps, m, l = _softmax([_nn2(_stack_heads(qp[c]), kv[c, 0])])
        return _pair(_nt2(ps[0], kv[c, 1])), _pair(m), _pair(l)


    def chip0():
        p = Prog()
        for nb in (1, 3):
            pl.semaphore_signal(bar, inc=1, device_id=(nb,), device_id_type=MESH)
        for n in ([("wqh", 1), ("x", 1), ("wqh", 0), ("x0a",)]
                  + [(j, c) for c in (A, C, D, B) for j in "kv"] + [("x0b",), ("wo",)]):
            ld(n).start()
        cast_wq(1)
        ldwait("x", 1)
        x1 = xf[1].astype(BF16)
        qp[D] = (_nn(x1, wqb[:, T:]) * QSCALE).astype(BF16)
        cast_wq(0)
        ldwait("x0a")
        qp[C] = (_nn(x1, wqb[:, :T]) * QSCALE).astype(BF16)
        q = qrows(xf[0, :NG])
        qp[A, :NG] = q[:, :T]
        qp[B, :NG] = q[:, T:]
        for c in (A, B, C, D):
            q0g[c] = qp[c, :NG]
        cast_kv(0, A)
        cast_kv(1, A)
        semwait(bar, 1)
        p.send(("q0", D), 1)
        p.send(("q0", C), 1)
        gsend[A] = _pack_glob(kv[A, 0], kv[A, 1])
        for k, t in enumerate(_pack96(kv[A, 0], kv[A, 1])):
            t96[k] = t
        semwait(ent, 1)
        p.send(("g", A), 3)
        p.send(("q0g",), 3)
        for c in (C, D, B):
            cast_kv(0, c)
            cast_kv(1, c)
        for c in (C, D):
            p.send(("L", 0, c), 1)
            p.send(("L", 1, c), 1)
        p.send(("gb",), 1)
        p.send(("t12",), 1)
        p.send(("t3",), 1)
        for c in (B, D, C):
            gsend[c] = _pack_glob(kv[c, 0], kv[c, 1])
        for c in (B, D, C):
            p.send(("g", c), 3)

        ldwait("x0b")
        q = qrows(xf[0, NG:])
        qp[A, NG:] = q[:, :T]
        qp[B, NG:] = q[:, T:]
        parts = {c: diag_only(c) for c in (C, D)}
        cast_wo()

        def front(c):
            qm = _stack_heads(qp[c])
            ps, m, l = _softmax([_nn2(qm, kv[c, 0]), masked(_nn2(qm, kvr[c, 0]), "right_g")])
            return ps[1], _pair(_nt2(ps[0], kv[c, 1])), _pair(m), _pair(l)

        def back(c, st):
            p1, acc, m, l = st
            parts[c] = (acc + _pair(_nt2(p1, kvr[c, 1])), m, l)

        p.recv(*[("Rp", A, n) for n in range(NP)])
        st = front(A)
        p.recv(("R", 1, A), ("R", 0, B))
        back(A, st)
        st = front(B)
        p.recv(("q", 1, B))
        helper(1, [(kv[B, 0], kv[B, 1], "left_g")])
        p.send(("rr",), 3)
        p.send(("st", 0), 1)
        p.send(("r", 0, 0), 1)
        p.send(("rm",), 1)
        p.recv(("R", 1, B))
        back(B, st)
        p.drain(keep=[("gb",), ("t12",), ("t3",), ("st", 0), ("r", 0, 0), ("rm",)])

        def with_chip1(c, lse_3, lse_1):
            acc, m, l = parts[c]
            w0, (w3, w1t) = _weights(m[:NG], l[:NG], [lse_3, lse_1[:NG]])
            top = acc[:NG] * w0 + w3 * o3[c].astype(F32)
            w0, (w1b,) = _weights(m[NG:], l[NG:], [lse_1[NG:]])
            return jnp.concatenate([top, acc[NG:] * w0], axis=0), jnp.concatenate([w1t, w1b], axis=0)

        p.recv(("lse3", 0), ("o3", D), ("o3", C), ("o3", A))
        l3 = _unfold(lse3[0], 3 * NG)
        acc, m, l = parts[A]
        w0, (w3,) = _weights(m[:NG], l[:NG], [l3[2 * NG:]])
        ca = jnp.concatenate([acc[:NG] * w0 + w3 * o3[A].astype(F32), acc[NG:] * (1.0 / l[NG:])], axis=0)
        acc_b, m_b, l_b = parts[B]
        cb = jnp.concatenate([jnp.zeros((NG, T), F32), acc_b[NG:] * (1.0 / l_b[NG:])], axis=0)
        oproj_both(0, ca, cb)
        p.recv(("r0d",), ("st10",))
        lse1 = _unfold(st10[...], 2 * T)
        base, w1 = with_chip1(D, l3[:NG], lse1[:T])
        oproj_first(D, base + w1 * r0[1].astype(F32))
        base, w1 = with_chip1(C, l3[NG:2 * NG], lse1[T:])
        p.recv(("lse3", 1))
        w0, (w3,) = _weights(m_b[:NG], l_b[:NG], [_unfold(lse3[1], NG)])
        top_b = acc_b[:NG] * w0
        p.recv(("r0c_hi",), ("r0c_lo",), ("o3", B))
        oproj_add(C, base + w1 * r0[0].astype(F32))
        out[0, :NG] = out[0, :NG] + _nn(top_b + w3 * o3[B].astype(F32), wo_rows(B))
        p.drain()

    def chip1():
        p = Prog()
        for nb in (0, 2):
            pl.semaphore_signal(bar, inc=1, device_id=(nb,), device_id_type=MESH)
        for n in ([("kp", A, n) for n in range(NP)] + [("v", A)] + [(j, c) for c in (B, C, D) for j in "kv"]
                  + [("wqh", 1), ("x", 0), ("wqh", 0), ("x", 1), ("wo",)]):
            ld(n).start()
        semwait(bar, 1)
        for n in range(NP):
            cast_k_part(A, n)
            p.send(("Rp", A, n), 0)
        for j, c in ((1, A), (0, B)):
            cast_kv(j, c)
            p.send(("R", j, c), 0)
        semwait(ent, 1)
        p.send(("L", 0, A), 2)
        p.send(("Lh", 0), 2)
        cast_kv(1, B)
        for c in (C, D):
            for j in (0, 1):
                cast_kv(j, c)
        cast_wq(1)
        ldwait("x", 0)
        qpair(B)
        p.send(("q", 1, B), 0)
        p.send(("q", 0, B), 2)
        p.send(("R", 1, B), 0)
        p.send(("Lh", 1), 2)
        p.send(("L", 0, C), 2)
        p.send(("L", 1, C), 2)
        cast_wq(0)
        ldwait("x", 1)
        qproj(1)

        neg = jnp.full((T - NG, T), NEG, F32)

        def c0_front(c, s1):
            s2g = _nn(_stack_heads(q0[c - C][:NG]), kvr[c, 0])
            s2 = jnp.concatenate([s2g[:NG], neg, s2g[NG:], neg], axis=0)
            ps, m, l = _softmax([s1, s2])
            p2 = jnp.concatenate([ps[1][:NG], ps[1][T:T + NG]], axis=0)
            return p2, _pair(_nt2(ps[0], kv[c, 1])), _pair(l), _pair(m + jnp.log2(l))

        def c0_scores(c):
            return masked(_nn2(_stack_heads(q0[c - C]), kv[c, 0]), "right_g")

        def c0_top(c, st):
            p2, acc, l, _ = st
            return norm(acc[:NG] + _pair(_nt(p2, kvr[c, 1])), l[:NG])

        p.recv(("q0", D), *[("Rp", D, n) for n in range(NP)])
        st_d = c0_front(D, c0_scores(D))
        r0[1, NG:] = norm(st_d[1][NG:], st_d[2][NG:])
        acc_b, m_b, l_b = diag_only(B)
        p.recv(("q0", C), ("R", 1, D))
        r0[1, :NG] = c0_top(D, st_d)
        s1_c = c0_scores(C)
        p.send(("r0d",), 0)
        qm_d = _stack_heads(qp[D])
        sd_d, sr_d = _nn2(qm_d, kv[D, 0]), masked(_nn2(qm_d, kvr[D, 0]), "right")
        qpair(A)
        cast_wo()
        p.recv(("R", 0, C))
        st_c = c0_front(C, s1_c)
        st10[...] = _fold(jnp.concatenate([st_d[3], st_c[3]], axis=0))
        r0[0, NG:] = norm(st_c[1][NG:], st_c[2][NG:])
        p.send(("st10",), 0)
        p.send(("r0c_hi",), 0)
        p.recv(("L", 0, C), ("L", 1, C))
        gsend[C] = _pack_glob(kvl[C, 0], kvl[C, 1])
        p.send(("g", C), 2)
        p.send(("L", 0, B), 2)
        p.send(("L", 1, B), 2)
        p.recv(("R", 1, C))
        r0[0, :NG] = c0_top(C, st_c)
        p.send(("r0c_lo",), 0)
        qm = _stack_heads(qp[C])
        ps, _, l = _softmax([
            _nn(qm, kv[C, 0]), masked(_nn(qm, kvr[C, 0]), "right"), masked(_nn2(qm, kvl[C, 0]), "left_g")])
        cc = norm(_pair(_nt(ps[0], kv[C, 1]) + _nt(ps[1], kvr[C, 1]) + _nt2(ps[2], kvl[C, 1])), _pair(l))
        p.recv(("L", 0, D), ("q", 1, D))
        ps_h, l_h = helper_front(1, [(kv[D, 0], "left"), (kvl[D, 0], "glob")])
        acc_h = _nt(ps_h[0], kv[D, 1])
        ps, _, l = _softmax([sd_d, sr_d, masked(_nn2(qm_d, kvl[D, 0]), "left_g")])
        acc = _nt(ps[0], kv[D, 1]) + _nt(ps[1], kvr[D, 1])
        oproj_first(C, cc)
        p.recv(("L", 1, D))
        rs[1] = norm(_pair(acc_h + _nt2(ps_h[1], kvl[D, 1])), l_h)
        cd = norm(_pair(acc + _nt2(ps[2], kvl[D, 1])), _pair(l))
        send_back(p, 1, 2)
        p.recv(("ga",), ("gb",))
        oproj_add(D, cd)
        kg, vg = _unpack_glob(gbuf[A])
        p.drain(keep=[("L", 1, B), ("st", 0), ("r", 0, 0), ("r", 0, 1)])
        p.recv(("R", 0, A), ("t12",))
        qm = _stack_heads(qp[A])
        k_l = _unpack96_k(t96[0], t96[1], kg)
        v_o = _unpack96_vo(t96[0], t96[1], vg)
        ps, _, l = _softmax([
            _nn(qm, kv[A, 0]), masked(_nn(qm, kvr[A, 0]), "right"), masked(_nn2(qm, k_l), "left_g")])
        acc = _pair(_nt2(ps[0], kv[A, 1]))
        p.recv(("t3",), ("st", 0), ("R", 1, A), ("st", 1))
        v_l = _unpack96_v(t96[2], v_o, vg)
        oproj_first(A, norm(acc + _pair(_nt2(ps[1], kvr[A, 1]) + _nt2(ps[2], v_l)), _pair(l)))
        w0, (wl, wr) = _weights(m_b, l_b, [peer_lse(0), peer_lse(1)])
        base = acc_b * w0
        p.recv(("r", 0, 0), ("r", 1, 0))
        merge_rows(B, 0, base, [(0, wl), (1, wr)])
        p.recv(("rm",), ("rf",), ("r2f",), ("r2m",))
        merge_rows(B, 1, base, [(0, wl), (1, wr)])
        p.drain()

    def chip2():
        p = Prog()
        first = [("kp", D, 0), ("kp", D, 1), ("kq", A, 0), ("kp", D, 2), ("kq", A, 1)]
        order = [(1, D), (1, A), (0, C), (0, B), (1, C), (1, B)]
        for n in (first + [("kv"[j], c) for j, c in order]
                  + [("wqh", 0), ("wqh", 1), ("x", 1), ("x", 0), ("wo",)]):
            ld(n).start()
        semwait(bar, 2)
        for nb in (1, 3):
            pl.semaphore_signal(ent, inc=1, device_id=(nb,), device_id_type=MESH)
        for kind, c, n in first:
            if kind == "kp":
                cast_k_part(c, n)
                p.send(("Rp", c, n), 1)
            else:
                cast_k_part2(c, n)
                p.send(("Lp", c, n), 3)
        for j, c in order:
            cast_kv(j, c)
            if c in (D, C):
                p.send(("R", j, c), 1)
            else:
                p.send(("L", j, c), 3)
        cast_wq(0, 1)
        ldwait("x", 1)
        qproj(1)
        p.send(("q", 1, D), 1)
        ldwait("x", 0)
        qproj(0)
        p.send(("q", 0, B), 3)
        cast_wo()

        def whole(c):
            qm = _stack_heads(qp[c])
            kg, vg = _unpack_glob(gbuf[c])
            ps, _, l = _softmax([
                _nn(qm, kv[c, 0]), masked(_nn(qm, kg), "glob"),
                masked(_nn(qm, kvl[c, 0]), "left"), masked(_nn(qm, kvr[c, 0]), "right")])
            acc = _nt(ps[0], kv[c, 1]) + _nt(ps[1], vg) + _nt(ps[2], kvl[c, 1]) + _nt(ps[3], kvr[c, 1])
            return norm(_pair(acc), _pair(l))

        def front(c, k, kind):
            qm = _stack_heads(qp[c])
            ps, m, l = _softmax([_nn(qm, kv[c, 0]), masked(_nn(qm, k), kind)])
            return ps[1], _pair(_nt2(ps[0], kv[c, 1])), _pair(m), _pair(l)

        def back(st, v, side):
            p1, acc, m, l = st
            w0, (w1,) = _weights(m, l, [peer_lse(side)])
            return (acc + _pair(_nt2(p1, v))) * w0, [(side, w1)]

        p.recv(("g", A))
        p.send(("ga",), 1)
        p.send(("R", 0, A), 1)
        p.send(("R", 1, A), 1)
        p.recv(("q", 0, B))
        helper(0, [(kv[B, 0], kv[B, 1], "right")])
        p.send(("r2r",), 3)
        p.send(("L", 0, D), 3)
        p.send(("L", 1, D), 3)
        p.send(("st", 1), 1)
        p.send(("r", 1, 0), 1)
        p.send(("r2m",), 1)
        p.recv(("L", 0, A), ("R", 0, A), ("R", 1, A), ("Lh", 0), ("Lh", 1))
        ca = whole(A)
        p.recv(("q", 1, C))
        helper(1, [(kv[C, 0], kv[C, 1], "left")])
        oproj_first(A, ca)
        send_back(p, 1, 3)
        p.drain(keep=[("R", 1, A), ("L", 1, D), ("st", 0), ("st", 1), ("r", 0, 0), ("r", 0, 1),
                      ("r", 1, 0), ("r2m",)])
        p.recv(("L", 0, C), ("R", 0, C), ("L", 1, C), ("R", 1, C), ("g", C))
        cc = whole(C)
        p.recv(("R", 0, D), ("L", 0, B))
        st_d = front(D, kvr[D, 0], "right")
        st_b = front(B, kvl[B, 0], "left")
        oproj_first(C, cc)
        p.recv(("R", 1, D), ("st", 1), ("L", 1, B), ("st", 0))
        base_d, parts_d = back(st_d, kvr[D, 1], 0)
        base_b, parts_b = back(st_b, kvl[B, 1], 1)
        p.drain()
        for h in (0, 1):
            p.recv(("r", 1, h), ("r", 0, h))
            merge_rows(B, h, base_b, parts_b)
            merge_rows(D, h, base_d, parts_d)

    def chip3():
        p = Prog()
        pl.semaphore_signal(bar, inc=1, device_id=(2,), device_id_type=MESH)
        semwait(bar, 1)
        pl.semaphore_signal(ent, inc=1, device_id=(0,), device_id_type=MESH)
        for n in ([(j, c) for c in (A, C, D, B) for j in "kv"]
                  + [("wqh", 0), ("wqh", 1), ("x", 1), ("x", 0), ("wo",)]):
            ld(n).start()
        for j in (0, 1):
            cast_kv(j, A)
        semwait(ent, 1)
        p.send(("R", 0, A), 2)
        p.send(("R", 1, A), 2)
        for c in (C, D, B):
            for j in (0, 1):
                cast_kv(j, c)
        cast_wq(0, 1)
        p.recv(("g", A))
        p.send(("gf", A), 2)
        ldwait("x", 1)
        qproj(1)
        p.send(("q", 1, C), 2)
        for c in (C, D):
            for j in (0, 1):
                p.send(("R", j, c), 2)
        ldwait("x", 0)
        qproj(0)

        def g_front(c, with_left):
            qm = _stack_heads(q0g[c])
            tiles = [_nn(qm, kv[c, 0])]
            if with_left:
                tiles.append(_nn(qm, kvl[c, 0]))
            ps, m, l = _softmax(tiles)
            return ps, _pair(_nt(ps[0], kv[c, 1])), _pair(l), _pair(m + jnp.log2(l))

        def g_back(c, st):
            ps, acc, l, _ = st
            if len(ps) > 1:
                acc = acc + _pair(_nt(ps[1], kvl[c, 1]))
            o3[c] = norm(acc, l)

        def front(c):
            qm = _stack_heads(qp[c])
            kg, vg = _unpack_glob(gbuf[c])
            ps, _, l = _softmax([
                _nn(qm, kv[c, 0]), masked(_nn(qm, kg), "glob"), masked(_nn2(qm, kvl[c, 0]), "left")])
            return ps[2], _pair(_nt2(ps[0], kv[c, 1]) + _nt2(ps[1], vg)), _pair(l)

        def back(c, st):
            p_l, acc, l = st
            return norm(acc + _pair(_nt2(p_l, kvl[c, 1])), l)

        p.recv(("q0g",), ("Lp", A, 0), ("Lp", A, 1))
        gd, gc, gst = g_front(D, False), g_front(C, False), g_front(A, True)
        g_back(D, gd)
        g_back(C, gc)
        lse3[0] = _fold(jnp.concatenate([gd[3], gc[3], gst[3]], axis=0))
        st = front(A)
        p.send(("lse3", 0), 0)
        p.send(("o3", D), 0)
        p.send(("o3", C), 0)
        p.recv(("L", 1, A))
        g_back(A, gst)
        ca = back(A, st)
        p.send(("o3", A), 0)
        p.recv(("g", B), ("L", 0, B))
        gst = g_front(B, True)
        lse3[1] = _fold(gst[3])
        st = front(B)
        p.send(("lse3", 1), 0)
        cast_wo()
        p.recv(("L", 1, B))
        g_back(B, gst)
        p.send(("o3", B), 0)
        p.recv(("g", D), ("g", C))
        oproj_both(0, ca, back(B, st))
        kg, vg = _unpack_glob(gbuf[C])
        qm = _stack_heads(qp[C])
        ps, m_c, l_c = _softmax([_nn(qm, kv[C, 0]), masked(_nn(qm, kg), "glob")])
        acc_c = _pair(_nt(ps[0], kv[C, 1]) + _nt(ps[1], vg))
        p.recv(("q", 0, B), ("r2r",), ("rr",))
        p.send(("rf",), 1)
        p.send(("r2f",), 1)
        kg, vg = _unpack_glob(gbuf[B])
        helper(0, [(kv[B, 0], kv[B, 1], "right"), (kg, vg, "glob")])
        send_back(p, 0, 2)
        p.recv(("L", 0, D))
        st = front(D)
        p.recv(("L", 1, D), ("st", 0))
        oproj_first(D, back(D, st))
        w0, (w1,) = _weights(_pair(m_c), _pair(l_c), [peer_lse(0)])
        base = acc_c * w0
        p.drain(keep=[("r", 1, 0), ("r", 1, 1)])
        for h in (0, 1):
            p.recv(("r", 0, h))
            merge_rows(C, h, base, [(0, w1)])
        p.drain()

    for c, prog in ((1, chip1), (2, chip2), (3, chip3), (0, chip0)):
        pl.when(me == c)(prog)


def pallas_dist_sparse_attn_localglobal_qseq_kvseq_b2_sq128_skv128_hq4_dh64_kernel(
    x: jax.Array,
    Wq: jax.Array,
    K_ext: jax.Array,
    V_ext: jax.Array,
    Wo: jax.Array,
):
    kt = jnp.transpose(K_ext, (0, 2, 3, 1)).reshape(4 * T, T)
    vt = jnp.transpose(V_ext, (0, 2, 3, 1)).reshape(4 * T, T)
    n_rc = 53
    any_spec = pl.BlockSpec(memory_space=pl.ANY)
    no_debug_checks = {
        k: True for k in ("disable_semaphore_checks", "disable_bounds_checks")
        if hasattr(pltpu.CompilerParams, k)}
    return pl.pallas_call(
        _body,
        out_shape=jax.ShapeDtypeStruct(x.shape, F32),
        in_specs=[any_spec] * 5,
        out_specs=pl.BlockSpec(memory_space=pltpu.VMEM),
        scratch_shapes=[
            pltpu.VMEM((2, T, 512), F32),
            pltpu.VMEM((2, 512, T), F32),
            pltpu.VMEM((256, 512), F32),
            pltpu.VMEM((4, 2, T, T), F32),
            pltpu.VMEM((512 // 2, 256), U32),
            pltpu.VMEM((256 // 2, 512), U32),
            pltpu.VMEM((4, 2, T // 2, T), U32),
            pltpu.VMEM((4, 2, T // 2, T), U32),
            pltpu.VMEM((4, 2, T // 2, T), U32),
            pltpu.VMEM((4, T // 2, T), U32),
            pltpu.VMEM((2, T // 2, T), U32),
            pltpu.VMEM((4, NG // 2, T), U32),
            pltpu.VMEM((4, 64 // 2, T), U32),
            pltpu.VMEM((4, 64 // 2, T), U32),
            pltpu.VMEM((8, T), F32),
            pltpu.VMEM((2, T // 2, T), U32),
            pltpu.VMEM((2, 8, T), F32),
            pltpu.VMEM((4, NG // 2, T), U32),
            pltpu.VMEM((3, 64 // 2, T), U32),
            pltpu.VMEM((2, T // 2, T), U32),
            pltpu.VMEM((2, 2, T), F32),
            pltpu.VMEM((2, 2, T), F32),
            pltpu.VMEM((2, T // 2, T), U32),
            pltpu.VMEM((2, T // 2, T), U32),
            pltpu.SemaphoreType.DMA((18,)),
            pltpu.SemaphoreType.DMA((n_rc,)),
            pltpu.SemaphoreType.DMA((n_rc,)),
            pltpu.SemaphoreType.REGULAR,
        ],
        compiler_params=pltpu.CompilerParams(collective_id=0, **no_debug_checks),
    )(x, Wq, kt, vt, Wo)
```
